```python
import numpy as np

kernel_name = "dist_max_ax1_xy_m2048_n1024"

def setup_inputs():
    return {"x": np.random.randn(4096, 2048).astype(np.float32)}

def reference(x: np.ndarray) -> np.ndarray:
    return np.max(x, axis=1, keepdims=True)
```

```python
import jax
import jax.numpy as jnp
from jax import lax
from jax.experimental import pallas as pl
from jax.experimental.pallas import tpu as pltpu

M, N = 2048, 1024
LANES, SUBLANES = 128, 8

SROWS = 48
CHUNKS = (848, 640, 128, 128, 128, 96, 32)
W_IN, W_OUT = 0, 3
SENDS = (1920, 2048)


def pallas_dist_max_ax1_xy_m2048_n1024_kernel(x: jax.Array):
    nch = len(CHUNKS)
    starts = [SROWS + sum(CHUNKS[:i]) for i in range(nch)]
    ns = len(SENDS)
    sstarts = [0] + list(SENDS[:-1])

    def body(x_hbm, out_ref, xbuf, sm, part, rbuf, in_sems, s_in, s_out,
             send_sems, recv_sems):
        my_x = lax.axis_index("x")
        my_y = lax.axis_index("y")
        nbr = (my_x, 1 - my_y)

        copies = [
            pltpu.make_async_copy(
                x_hbm.at[pl.ds(starts[c], CHUNKS[c]), :],
                xbuf.at[pl.ds(starts[c], CHUNKS[c]), :],
                in_sems.at[c])
            for c in range(nch)
        ]
        to_smem = pltpu.make_async_copy(x_hbm.at[pl.ds(0, SROWS), :], sm, s_in)
        from_smem = pltpu.make_async_copy(sm, xbuf.at[pl.ds(0, SROWS), :], s_out)
        copies[0].start()
        to_smem.start()
        for cp in copies[1:]:
            cp.start()

        bar = pltpu.get_barrier_semaphore()
        pl.semaphore_signal(bar, inc=1, device_id=nbr,
                            device_id_type=pl.DeviceIdType.MESH)

        def rdma(k):
            sl = pl.ds(sstarts[k], SENDS[k] - sstarts[k])
            return pltpu.make_async_remote_copy(
                src_ref=part.at[:, sl], dst_ref=rbuf.at[:, sl],
                send_sem=send_sems.at[k], recv_sem=recv_sems.at[k],
                device_id=nbr, device_id_type=pl.DeviceIdType.MESH)

        diff = (lax.broadcasted_iota(jnp.int32, (SUBLANES, LANES), 1)
                - lax.broadcasted_iota(jnp.int32, (SUBLANES, LANES), 0))
        accs = {}

        def rows8(r):
            ms = [xbuf[pl.ds(r, SUBLANES), pl.ds(j * LANES, LANES)]
                  for j in range(N // LANES)]
            while len(ms) > 1:
                ms = [jnp.maximum(ms[2 * i], ms[2 * i + 1])
                      for i in range(len(ms) // 2)]
            v = jnp.max(ms[0], axis=1, keepdims=True)
            g = r // LANES
            acc, n = accs.get(g, (None, 0))
            vb = jnp.broadcast_to(v, (SUBLANES, LANES))
            acc = jnp.where(diff == (r % LANES), vb,
                            -jnp.inf if acc is None else acc)
            n += SUBLANES
            if n == LANES:
                part[:, pl.ds(g * LANES, LANES)] = jnp.max(acc, axis=0,
                                                           keepdims=True)
                acc = None
            accs[g] = (acc, n)

        k = 0
        for c in range(nch):
            copies[c].wait()
            for r in range(starts[c], starts[c] + CHUNKS[c], SUBLANES):
                rows8(r)
            if c == W_IN:
                to_smem.wait()
                from_smem.start()
            if c == W_OUT:
                from_smem.wait()
                for r in range(0, SROWS, SUBLANES):
                    rows8(r)
            while k < ns and all(
                    accs.get(g, (None, 0))[1] == LANES
                    for g in range(sstarts[k] // LANES, SENDS[k] // LANES)):
                if k == 0:
                    pl.semaphore_wait(bar, 1)
                rdma(k).start()
                k += 1
        assert k == ns

        for k in range(ns):
            sl = pl.ds(sstarts[k], SENDS[k] - sstarts[k])
            rdma(k).wait_recv()
            out_ref[:, sl] = jnp.maximum(part[:, sl], rbuf[:, sl])
        for k in range(ns):
            rdma(k).wait_send()

    out = pl.pallas_call(
        body,
        out_shape=jax.ShapeDtypeStruct((1, M), jnp.float32),
        in_specs=[pl.BlockSpec(memory_space=pl.ANY)],
        out_specs=pl.BlockSpec(memory_space=pltpu.VMEM),
        scratch_shapes=[
            pltpu.VMEM((M, N), jnp.float32),
            pltpu.SMEM((SROWS, N), jnp.float32),
            pltpu.VMEM((1, M), jnp.float32),
            pltpu.VMEM((1, M), jnp.float32),
            pltpu.SemaphoreType.DMA((nch,)),
            pltpu.SemaphoreType.DMA,
            pltpu.SemaphoreType.DMA,
            pltpu.SemaphoreType.DMA((ns,)),
            pltpu.SemaphoreType.DMA((ns,)),
        ],
        compiler_params=pltpu.CompilerParams(
            collective_id=0,
            vmem_limit_bytes=32 * 1024 * 1024,
            disable_bounds_checks=True,
            disable_semaphore_checks=True,
        ),
    )(x)
    return out.reshape(M, 1)
```

```python
import jax
import jax.numpy as jnp
from jax import lax
from jax.experimental import pallas as pl
from jax.experimental.pallas import tpu as pltpu

M, N = 2048, 1024
LANES, SUB = 128, 8
SLOTS = 16
NEG = -jnp.inf

N_MAIN = 2 * SLOTS
WINDOW = 16
PRE = 6
TAIL_AT = 20
TAIL = ((0, 12), (12, 4))
RAW = ((1, 10), (11, 4), (15, 1))
G_TAIL, G_RAW = 14, 15


def pallas_dist_max_ax1_xy_m2048_n1024_kernel(x: jax.Array):
    def body(x_hbm, out_ref, xbuf, rawbuf, part, rpart, tmsg, rtmsg,
             main_sems, tail_sems, first_sem, reread_sem,
             send_sems, recv_sems, raw_send_sems, raw_recv_sems):
        nbr = (lax.axis_index("x"), 1 - lax.axis_index("y"))

        def main_copy(c):
            b5, slot = divmod(c, SLOTS)
            hi = pl.ds(0, 4 - b5)
            return pltpu.make_async_copy(
                x_hbm.at[hi, b5, :, slot], xbuf.at[hi, b5, :, slot],
                main_sems.at[c])

        def run_copy(b4, slot0, n, sem):
            return pltpu.make_async_copy(
                x_hbm.at[3, 1, b4, pl.ds(slot0, n)],
                xbuf.at[3, 1, b4, pl.ds(slot0, n)], sem)

        def raw_copy(i):
            slot0, n = RAW[i]
            return pltpu.make_async_remote_copy(
                src_ref=x_hbm.at[3, 1, 1, pl.ds(slot0, n)],
                dst_ref=rawbuf.at[pl.ds(slot0, n)],
                send_sem=raw_send_sems.at[i], recv_sem=raw_recv_sems.at[i],
                device_id=nbr, device_id_type=pl.DeviceIdType.MESH)

        def msg_copy(k):
            src, dst = ((part, rpart), (tmsg, rtmsg))[k]
            return pltpu.make_async_remote_copy(
                src_ref=src, dst_ref=dst,
                send_sem=send_sems.at[k], recv_sem=recv_sems.at[k],
                device_id=nbr, device_id_type=pl.DeviceIdType.MESH)

        first = run_copy(1, 0, 1, first_sem)
        tails = [run_copy(0, s0, n, tail_sems.at[w])
                 for w, (s0, n) in enumerate(TAIL)]
        reread = run_copy(1, 1, SLOTS - 1, reread_sem)

        first.start()
        main_copy(0).start()
        barrier = pltpu.get_barrier_semaphore()
        pl.semaphore_signal(barrier, inc=1, device_id=nbr,
                            device_id_type=pl.DeviceIdType.MESH)
        for c in range(1, PRE):
            main_copy(c).start()
        pl.semaphore_wait(barrier, 1)
        for i in range(len(RAW)):
            raw_copy(i).start()
        for c in range(PRE, WINDOW):
            main_copy(c).start()

        diag = (lax.broadcasted_iota(jnp.int32, (SUB, LANES), 1)
                - lax.broadcasted_iota(jnp.int32, (SUB, LANES), 0))

        def row_max(block_ref):
            vs = [block_ref[:, pl.ds(j * LANES, LANES)] for j in range(N // LANES)]
            while len(vs) > 1:
                vs = [jnp.maximum(vs[2 * i], vs[2 * i + 1])
                      for i in range(len(vs) // 2)]
            return jnp.broadcast_to(jnp.max(vs[0], axis=1, keepdims=True),
                                    (SUB, LANES))

        def place(acc, slot, v):
            return jnp.where(diag == slot * SUB, v, NEG if acc is None else acc)

        def collapse(acc):
            return jnp.max(acc, axis=0, keepdims=True)

        accs = {}
        for c in range(N_MAIN):
            b5, slot = divmod(c, SLOTS)
            main_copy(c).wait()
            if c + WINDOW < N_MAIN:
                main_copy(c + WINDOW).start()
            if c == TAIL_AT:
                for cp in tails:
                    cp.start()
            for hi in range(4 - b5):
                for b4 in range(2):
                    g = hi * 4 + b5 * 2 + b4
                    accs[g] = place(accs.get(g), slot,
                                    row_max(xbuf.at[hi, b5, b4, slot]))
                    if slot == SLOTS - 1:
                        part[:, pl.ds(g * LANES, LANES)] = collapse(accs.pop(g))
            if c == TAIL_AT:
                first.wait()
                part[:, pl.ds(G_TAIL * LANES, LANES)] = collapse(
                    place(None, 0, row_max(xbuf.at[3, 1, 1, 0])))
        msg_copy(0).start()

        acc = None
        for w, (s0, n) in enumerate(TAIL):
            tails[w].wait()
            for s in range(s0, s0 + n):
                acc = place(acc, s, row_max(xbuf.at[3, 1, 0, s]))
        tail_max = collapse(acc)
        tmsg[...] = tail_max
        msg_copy(1).start()

        reread.start()
        theirs = None
        for i, (s0, n) in enumerate(RAW):
            raw_copy(i).wait_recv()
            for s in range(s0, s0 + n):
                theirs = place(theirs, s, row_max(rawbuf.at[s]))
            if i == 0:
                reread.wait()
                mine = None
                for s in range(1, SLOTS):
                    mine = place(mine, s, row_max(xbuf.at[3, 1, 1, s]))
        raw_max = collapse(jnp.maximum(mine, theirs))

        msg_copy(0).wait_recv()
        bulk = pl.ds(0, G_TAIL * LANES)
        out_ref[:, bulk] = jnp.maximum(part[:, bulk], rpart[:, bulk])
        extra = pl.ds(G_TAIL * LANES, LANES)
        out_ref[:, pl.ds(G_RAW * LANES, LANES)] = jnp.maximum(
            raw_max, jnp.maximum(part[:, extra], rpart[:, extra]))

        for k in range(2):
            msg_copy(k).wait_send()
        for i in range(len(RAW)):
            raw_copy(i).wait_send()
        msg_copy(1).wait_recv()
        out_ref[:, pl.ds(G_TAIL * LANES, LANES)] = jnp.maximum(tail_max, rtmsg[...])

    out = pl.pallas_call(
        body,
        out_shape=jax.ShapeDtypeStruct((1, M), jnp.float32),
        in_specs=[pl.BlockSpec(memory_space=pl.ANY)],
        out_specs=pl.BlockSpec(memory_space=pltpu.VMEM),
        scratch_shapes=[
            pltpu.VMEM((4, 2, 2, SLOTS, SUB, N), jnp.float32),
            pltpu.VMEM((SLOTS, SUB, N), jnp.float32),
            pltpu.VMEM((1, M - LANES), jnp.float32),
            pltpu.VMEM((1, M - LANES), jnp.float32),
            pltpu.VMEM((1, LANES), jnp.float32),
            pltpu.VMEM((1, LANES), jnp.float32),
            pltpu.SemaphoreType.DMA((N_MAIN,)),
            pltpu.SemaphoreType.DMA((len(TAIL),)),
            pltpu.SemaphoreType.DMA,
            pltpu.SemaphoreType.DMA,
            pltpu.SemaphoreType.DMA((2,)),
            pltpu.SemaphoreType.DMA((2,)),
            pltpu.SemaphoreType.DMA((len(RAW),)),
            pltpu.SemaphoreType.DMA((len(RAW),)),
        ],
        compiler_params=pltpu.CompilerParams(
            collective_id=0,
            vmem_limit_bytes=32 * 1024 * 1024,
            disable_bounds_checks=True,
            disable_semaphore_checks=True,
        ),
    )(x.reshape(4, 2, 2, SLOTS, SUB, N))
    return out.reshape(M, 1)
```

```python
import jax
import jax.numpy as jnp
from jax import lax
from jax.experimental import pallas as pl
from jax.experimental.pallas import tpu as pltpu

M, N = 2048, 1024
LANES, SUB, SLOTS = 128, 8, 16
TILES = N // LANES
NEG = -jnp.inf

N_MAIN = 2 * SLOTS
PRE = 2
WINDOW = 6
G_TAIL, G_RAW = 14, 15

N_SMEM = 6
SMEM_IN_AT, SMEM_OUT_AT = 10, 26
TAIL = ((6, 6), (12, 3), (15, 1))
LAST0 = TAIL[1][0]

CUT = 6
HEAD = ((0, 1, 0, TILES), (1, 1, CUT, TILES - CUT))
RAW = ((1, 1, 0, CUT), (2, 13, 0, TILES), (15, 1, 0, TILES))

BULK, EARLY, LAST, BACK = range(4)


def pallas_dist_max_ax1_xy_m2048_n1024_kernel(x: jax.Array):
    def body(x_hbm, out_ref, xbuf, rawbuf, bounce, part, rpart, small, rsmall,
             rlast, main_sems, head_sems, tail_sems, reread_sems, smem_sems,
             send_sems, recv_sems, raw_send_sems, raw_recv_sems):
        my_y = lax.axis_index("y")
        nbr = (lax.axis_index("x"), 1 - my_y)
        tail_hbm, raw_hbm = x_hbm.at[3, 1, 0], x_hbm.at[3, 1, 1]
        tail_buf, raw_buf = xbuf.at[3, 1, 0], xbuf.at[3, 1, 1]

        def main_copy(c):
            b5, slot = divmod(c, SLOTS)
            hi = pl.ds(0, 4 - b5)
            return pltpu.make_async_copy(
                x_hbm.at[hi, b5, :, slot], xbuf.at[hi, b5, :, slot],
                main_sems.at[c])

        def piece(group_ref, slot0, n, tile0=0, n_tiles=TILES):
            return group_ref.at[pl.ds(slot0, n), :,
                                pl.ds(tile0 * LANES, n_tiles * LANES)]

        def local(src, dst, pieces, sems):
            return [pltpu.make_async_copy(piece(src, *p), piece(dst, *p),
                                          sems.at[i])
                    for i, p in enumerate(pieces)]

        def remote(src, dst, send_sem, recv_sem):
            return pltpu.make_async_remote_copy(
                src_ref=src, dst_ref=dst, send_sem=send_sem, recv_sem=recv_sem,
                device_id=nbr, device_id_type=pl.DeviceIdType.MESH)

        def raw_copy(i):
            return remote(piece(raw_hbm, *RAW[i]), piece(rawbuf, *RAW[i]),
                          raw_send_sems.at[i], raw_recv_sems.at[i])

        def msg(k):
            src, dst = {
                BULK: (part, rpart),
                EARLY: (small.at[0], rsmall.at[0]),
                LAST: (small.at[1], rlast),
                BACK: (small.at[2], rsmall.at[1]),
            }[k]
            return remote(src, dst, send_sems.at[k], recv_sems.at[k])

        heads = local(raw_hbm, raw_buf, HEAD, head_sems)
        rereads = local(raw_hbm, raw_buf, RAW, reread_sems)
        tails = local(tail_hbm, tail_buf, TAIL, tail_sems)
        to_smem = pltpu.make_async_copy(
            tail_hbm.at[pl.ds(0, N_SMEM)], bounce, smem_sems.at[0])
        from_smem = pltpu.make_async_copy(
            bounce, tail_buf.at[pl.ds(0, N_SMEM)], smem_sems.at[1])

        for cp in heads:
            cp.start()
        main_copy(0).start()
        to_smem.start()
        barrier = pltpu.get_barrier_semaphore()
        pl.semaphore_signal(barrier, inc=1, device_id=nbr,
                            device_id_type=pl.DeviceIdType.MESH)
        for c in range(1, PRE):
            main_copy(c).start()

        @pl.when(my_y == 1)
        def _():
            pl.semaphore_wait(barrier, 1)
            for i in range(len(RAW)):
                raw_copy(i).start()

        for c in range(PRE, WINDOW):
            main_copy(c).start()

        diag = (lax.broadcasted_iota(jnp.int32, (SUB, LANES), 1)
                - lax.broadcasted_iota(jnp.int32, (SUB, LANES), 0))

        def fold(block_ref, tile0=0, n_tiles=TILES):
            vs = [block_ref[:, pl.ds(j * LANES, LANES)]
                  for j in range(tile0, tile0 + n_tiles)]
            while len(vs) > 1:
                vs = [jnp.maximum(*vs[i:i + 2]) if i + 1 < len(vs) else vs[i]
                      for i in range(0, len(vs), 2)]
            return vs[0]

        def place(acc, slot, folded):
            v = jnp.broadcast_to(jnp.max(folded, axis=1, keepdims=True),
                                 (SUB, LANES))
            return jnp.where(diag == slot * SUB, v, NEG if acc is None else acc)

        def collapse(acc):
            return jnp.max(acc, axis=0, keepdims=True)

        def reduce_piece(acc, group_ref, slot0, n, tile0=0, n_tiles=TILES):
            for s in range(slot0, slot0 + n):
                acc = place(acc, s, fold(group_ref.at[s], tile0, n_tiles))
            return acc

        accs = {}
        for c in range(N_MAIN):
            b5, slot = divmod(c, SLOTS)
            main_copy(c).wait()
            if c + WINDOW < N_MAIN:
                main_copy(c + WINDOW).start()
            elif c + WINDOW == N_MAIN:
                for cp in tails:
                    cp.start()
            for hi in range(4 - b5):
                for b4 in range(2):
                    g = hi * 4 + b5 * 2 + b4
                    accs[g] = place(accs.get(g), slot,
                                    fold(xbuf.at[hi, b5, b4, slot]))
                    if slot == SLOTS - 1:
                        part[:, pl.ds(g * LANES, LANES)] = collapse(accs.pop(g))
            if c == SMEM_IN_AT:
                to_smem.wait()
                from_smem.start()
            if c == SLOTS - 1:
                acc = None
                for cp, p in zip(heads, HEAD):
                    cp.wait()
                    acc = reduce_piece(acc, raw_buf, *p)
                part[:, pl.ds(G_TAIL * LANES, LANES)] = collapse(acc)

                @pl.when(my_y == 0)
                def _():
                    pl.semaphore_wait(barrier, 1)
            if c == SMEM_OUT_AT:
                from_smem.wait()
                accs[G_TAIL] = reduce_piece(None, tail_buf, 0, N_SMEM)
        msg(BULK).start()

        tails[0].wait()
        early = collapse(reduce_piece(accs.pop(G_TAIL), tail_buf, *TAIL[0]))
        small[0] = early
        msg(EARLY).start()
        folded = []
        for cp, (slot0, n) in zip(tails[1:], TAIL[1:]):
            cp.wait()
            folded += [fold(tail_buf.at[s]) for s in range(slot0, slot0 + n)]
        acc = None
        for s, v in enumerate(folded, LAST0):
            acc = place(acc, s, v)
        last = collapse(acc)
        small[1] = last
        msg(LAST).start()

        for cp in rereads:
            cp.start()
        for cp in rereads:
            cp.wait()
        mine = collapse(reduce_piece(None, raw_buf, 0, SLOTS))

        @pl.when(my_y == 0)
        def _():
            small[2] = mine
            msg(BACK).start()
            acc = None
            for i, p in enumerate(RAW):
                raw_copy(i).wait_recv()
                acc = reduce_piece(acc, rawbuf, *p)
            rsmall[1] = collapse(acc)
            msg(BACK).wait_send()

        @pl.when(my_y == 1)
        def _():
            for i in range(len(RAW)):
                raw_copy(i).wait_send()
            msg(BACK).wait_recv()

        for k in (BULK, EARLY, LAST):
            msg(k).wait_send()

        msg(BULK).wait_recv()
        bulk = pl.ds(0, G_TAIL * LANES)
        out_ref[:, bulk] = jnp.maximum(part[:, bulk], rpart[:, bulk])
        out_ref[:, pl.ds(G_RAW * LANES, LANES)] = jnp.maximum(
            jnp.maximum(mine, rsmall[1]),
            rpart[:, pl.ds(G_TAIL * LANES, LANES)])

        msg(EARLY).wait_recv()
        known = jnp.maximum(jnp.maximum(early, last), rsmall[0])
        lane = lax.broadcasted_iota(jnp.int32, (1, LANES), 1)
        msg(LAST).wait_recv()
        theirs = known
        for l in range(LAST0 * SUB, LANES):
            theirs = jnp.where(lane == l, rlast[0, l], theirs)
        out_ref[:, pl.ds(G_TAIL * LANES, LANES)] = jnp.maximum(known, theirs)

    out = pl.pallas_call(
        body,
        out_shape=jax.ShapeDtypeStruct((1, M), jnp.float32),
        in_specs=[pl.BlockSpec(memory_space=pl.ANY)],
        out_specs=pl.BlockSpec(memory_space=pltpu.VMEM),
        scratch_shapes=[
            pltpu.VMEM((4, 2, 2, SLOTS, SUB, N), jnp.float32),
            pltpu.VMEM((SLOTS, SUB, N), jnp.float32),
            pltpu.SMEM((N_SMEM, SUB, N), jnp.float32),
            pltpu.VMEM((1, M - LANES), jnp.float32),
            pltpu.VMEM((1, M - LANES), jnp.float32),
            pltpu.VMEM((3, 1, LANES), jnp.float32),
            pltpu.VMEM((2, 1, LANES), jnp.float32),
            pltpu.SMEM((1, LANES), jnp.float32),
            pltpu.SemaphoreType.DMA((N_MAIN,)),
            pltpu.SemaphoreType.DMA((len(HEAD),)),
            pltpu.SemaphoreType.DMA((len(TAIL),)),
            pltpu.SemaphoreType.DMA((len(RAW),)),
            pltpu.SemaphoreType.DMA((2,)),
            pltpu.SemaphoreType.DMA((4,)),
            pltpu.SemaphoreType.DMA((4,)),
            pltpu.SemaphoreType.DMA((len(RAW),)),
            pltpu.SemaphoreType.DMA((len(RAW),)),
        ],
        compiler_params=pltpu.CompilerParams(
            collective_id=0,
            vmem_limit_bytes=32 * 1024 * 1024,
            disable_semaphore_checks=True,
        ),
    )(x.reshape(4, 2, 2, SLOTS, SUB, N))
    return out.reshape(M, 1)
```

```python
import jax
import jax.numpy as jnp
from jax import lax
from jax.experimental import pallas as pl
from jax.experimental.pallas import tpu as pltpu

M, N = 2048, 1024
LANES, SUB, SLOTS = 128, 8, 16
TILES = N // LANES
GT = SLOTS * TILES
NT = M * N // (SUB * LANES)
NEG = -jnp.inf

OFF, UNIT = 7, 16
PHASES = ((0, 1, 2, 3, 4, 5, 6), (7, 8, 9, 10, 11, 12, 13))
PRE = 1
WINDOW = 3
G_TAIL, G_RAW = 14, 15

SMEM_END = 55
SMEM_IN_AT, SMEM_OUT_AT = 6, 14
TAIL = (96, 120, 128)
HEAD_T = 12
HEAD_AT = 2
RAW = (120, 128)

BULK, EARLY, LAST, BACK = range(4)


def pallas_dist_max_ax1_xy_m2048_n1024_kernel(x: jax.Array):
    per = GT // UNIT
    steps = [(gs, u) for gs in PHASES for u in range(per)]
    n_main = len(steps)
    T0, R0 = G_TAIL * GT, G_RAW * GT
    tail_p = list(zip((SMEM_END,) + TAIL, TAIL))
    raw_p = list(zip((HEAD_T,) + RAW, RAW))
    last0 = TAIL[0] // TILES
    arrive = {}
    for c, (gs, u) in enumerate(steps):
        for g in gs:
            for t in range(g * GT + OFF + u * UNIT, g * GT + OFF + (u + 1) * UNIT):
                arrive[t] = c
    head_step = n_main // 2 - 1
    for t in range(OFF):
        arrive[t] = head_step
    ready = {}
    for g in range(G_TAIL):
        for s in range(SLOTS):
            c = max(arrive[g * GT + s * TILES + j] for j in range(TILES))
            ready.setdefault(c, []).append((g, s))

    def body(x_hbm, out_ref, xbuf, rawbuf, bounce, part, rpart, small, rsmall,
             rlast, main_sems, tail_sems, misc_sems,
             send_sems, recv_sems, raw_send_sems, raw_recv_sems):
        my_y = lax.axis_index("y")
        nbr = (lax.axis_index("x"), 1 - my_y)

        def span(t0, t1):
            return pl.ds(t0, t1 - t0)

        def local(t0, t1, sem):
            return pltpu.make_async_copy(x_hbm.at[span(t0, t1)], xbuf.at[span(t0, t1)], sem)

        def main_copies(c):
            gs, u = steps[c]
            return [local(g * GT + OFF + u * UNIT, g * GT + OFF + (u + 1) * UNIT, main_sems.at[c]) for g in gs]

        def remote(src, dst, send_sem, recv_sem):
            return pltpu.make_async_remote_copy(
                src_ref=src, dst_ref=dst, send_sem=send_sem, recv_sem=recv_sem,
                device_id=nbr, device_id_type=pl.DeviceIdType.MESH)

        def raw_copy(i):
            a, b = raw_p[i]
            return remote(x_hbm.at[span(R0 + a, R0 + b)], rawbuf.at[span(a, b)],
                          raw_send_sems.at[i], raw_recv_sems.at[i])

        def msg(k):
            src, dst = {
                BULK: (part, rpart),
                EARLY: (small.at[0], rsmall.at[0]),
                LAST: (small.at[1], rlast),
                BACK: (small.at[2], rsmall.at[1]),
            }[k]
            return remote(src, dst, send_sems.at[k], recv_sems.at[k])

        heads = [local(R0, R0 + HEAD_T, misc_sems.at[0]), local(0, OFF, misc_sems.at[4])]
        reread = local(R0 + HEAD_T, NT, misc_sems.at[1])
        tails = [local(T0 + a, T0 + b, tail_sems.at[i]) for i, (a, b) in enumerate(tail_p)]
        sm_span = span(T0 + OFF, T0 + SMEM_END)
        to_smem = pltpu.make_async_copy(x_hbm.at[sm_span], bounce, misc_sems.at[2])
        from_smem = pltpu.make_async_copy(bounce, xbuf.at[sm_span], misc_sems.at[3])

        if HEAD_AT is None:
            for cp in heads:
                cp.start()
        for i, cp in enumerate(main_copies(0)):
            cp.start()
            if i == 1:
                to_smem.start()
        barrier = pltpu.get_barrier_semaphore()
        pl.semaphore_signal(barrier, inc=1, device_id=nbr, device_id_type=pl.DeviceIdType.MESH)
        for c in range(1, PRE):
            for cp in main_copies(c):
                cp.start()

        @pl.when(my_y == 1)
        def _():
            pl.semaphore_wait(barrier, 1)
            for i in range(len(RAW)):
                raw_copy(i).start()

        for c in range(PRE, WINDOW):
            for cp in main_copies(c):
                cp.start()

        diag = (lax.broadcasted_iota(jnp.int32, (SUB, LANES), 1)
                - lax.broadcasted_iota(jnp.int32, (SUB, LANES), 0))

        def fold(ref, t0, t1):
            tiles = ref[span(t0, t1)]
            vs = [tiles[j] for j in range(t1 - t0)]
            while len(vs) > 1:
                vs = [jnp.maximum(*vs[i:i + 2]) if i + 1 < len(vs) else vs[i]
                      for i in range(0, len(vs), 2)]
            return vs[0]

        def fold_span(ref, base, t0, t1):
            return [(s, fold(ref, base + max(t0, s * TILES), base + min(t1, (s + 1) * TILES)))
                    for s in range(t0 // TILES, pl.cdiv(t1, TILES))]

        def place(acc, folded):
            for s, v in folded:
                acc = jnp.where(diag == s * SUB, jnp.max(v, axis=-1, keepdims=True),
                                NEG if acc is None else acc)
            return acc

        def collapse(acc):
            return jnp.max(acc, axis=-2, keepdims=True)

        accs, cnt = {}, {}
        for c in range(n_main):
            for cp in main_copies(c):
                cp.wait()
            if c + WINDOW < n_main:
                for cp in main_copies(c + WINDOW):
                    cp.start()
            elif c + WINDOW == n_main:
                for cp in tails:
                    cp.start()
            if c == HEAD_AT:
                for cp in heads:
                    cp.start()
            if c == head_step:
                for cp in heads:
                    cp.wait()
            for g, s in ready.get(c, []):
                accs[g] = place(accs.get(g), fold_span(xbuf, g * GT, s * TILES, (s + 1) * TILES))
                cnt[g] = cnt.get(g, 0) + 1
                if cnt[g] == SLOTS:
                    part[:, pl.ds(g * LANES, LANES)] = collapse(accs.pop(g))
            if c == SMEM_IN_AT:
                to_smem.wait()
                from_smem.start()
            if c == head_step:
                part[:, pl.ds(G_TAIL * LANES, LANES)] = collapse(place(None, fold_span(xbuf, R0, 0, HEAD_T)))

                @pl.when(my_y == 0)
                def _():
                    pl.semaphore_wait(barrier, 1)
            if c == SMEM_OUT_AT:
                from_smem.wait()
                acc = place(None, fold_span(xbuf, T0, TILES, SMEM_END // TILES * TILES))
        msg(BULK).start()

        tails[0].wait()
        early = collapse(place(acc, fold_span(xbuf, T0, 0, TILES)
                               + fold_span(xbuf, T0, SMEM_END // TILES * TILES, last0 * TILES)))
        small[0] = early
        msg(EARLY).start()
        folded = {}
        lo = last0 * TILES
        for cp, (_, t1) in zip(tails[1:], tail_p[1:]):
            cp.wait()
            for s, v in fold_span(xbuf, T0, lo, t1):
                folded[s] = jnp.maximum(folded[s], v) if s in folded else v
            lo = t1
        last = collapse(place(None, folded.items()))
        small[1] = last
        msg(LAST).start()

        reread.start()
        reread.wait()
        mine = collapse(place(None, fold_span(xbuf, R0, 0, GT)))

        @pl.when(my_y == 0)
        def _():
            small[2] = mine
            msg(BACK).start()
            acc = None
            for i, p in enumerate(raw_p):
                raw_copy(i).wait_recv()
                acc = place(acc, fold_span(rawbuf, 0, *p))
            rsmall[1] = collapse(acc)
            msg(BACK).wait_send()

        @pl.when(my_y == 1)
        def _():
            for i in range(len(RAW)):
                raw_copy(i).wait_send()
            msg(BACK).wait_recv()

        for k in (BULK, EARLY, LAST):
            msg(k).wait_send()

        msg(BULK).wait_recv()
        bulk = pl.ds(0, G_TAIL * LANES)
        out_ref[:, bulk] = jnp.maximum(part[:, bulk], rpart[:, bulk])
        out_ref[:, pl.ds(G_RAW * LANES, LANES)] = jnp.maximum(
            jnp.maximum(mine, rsmall[1]), rpart[:, pl.ds(G_TAIL * LANES, LANES)])

        msg(EARLY).wait_recv()
        known = jnp.maximum(jnp.maximum(early, last), rsmall[0])
        lane = lax.broadcasted_iota(jnp.int32, (1, LANES), 1)
        msg(LAST).wait_recv()
        theirs = known
        for l in range(last0 * SUB, LANES):
            theirs = jnp.where(lane == l, rlast[0, l], theirs)
        out_ref[:, pl.ds(G_TAIL * LANES, LANES)] = jnp.maximum(known, theirs)

    shape = (NT, SUB, LANES)
    x_tiles = x.reshape(M // SUB, SUB, TILES, LANES).transpose(0, 2, 1, 3).reshape(shape)
    out = pl.pallas_call(
        body,
        out_shape=jax.ShapeDtypeStruct((1, M), jnp.float32),
        in_specs=[pl.BlockSpec(memory_space=pl.ANY)],
        out_specs=pl.BlockSpec(memory_space=pltpu.VMEM),
        scratch_shapes=[
            pltpu.VMEM(shape, jnp.float32),
            pltpu.VMEM((GT, SUB, LANES), jnp.float32),
            pltpu.SMEM((SMEM_END - OFF, SUB, LANES), jnp.float32),
            pltpu.VMEM((1, M - LANES), jnp.float32),
            pltpu.VMEM((1, M - LANES), jnp.float32),
            pltpu.VMEM((3, 1, LANES), jnp.float32),
            pltpu.VMEM((2, 1, LANES), jnp.float32),
            pltpu.SMEM((1, LANES), jnp.float32),
            pltpu.SemaphoreType.DMA((n_main,)),
            pltpu.SemaphoreType.DMA((len(TAIL),)),
            pltpu.SemaphoreType.DMA((5,)),
            pltpu.SemaphoreType.DMA((4,)),
            pltpu.SemaphoreType.DMA((4,)),
            pltpu.SemaphoreType.DMA((len(RAW),)),
            pltpu.SemaphoreType.DMA((len(RAW),)),
        ],
        compiler_params=pltpu.CompilerParams(
            collective_id=0,
            vmem_limit_bytes=32 * 1024 * 1024,
            disable_semaphore_checks=True,
        ),
    )(x_tiles)
    return out.reshape(M, 1)
```

```python
import jax
import jax.numpy as jnp
from jax import lax
from jax.experimental import pallas as pl
from jax.experimental.pallas import tpu as pltpu

M, N = 2048, 1024
LANES, SUB = 128, 8
TILES = N // LANES
SLOTS = LANES // SUB
GT = SLOTS * TILES
GROUPS = M // LANES
NEG = -jnp.inf

OFF, UNIT, WAYS = 7, 16, 7
STEPS = [(g0, u) for g0 in (0, WAYS) for u in range(GT // UNIT)]
WINDOW = 3
G_TAIL = 14
SMEM = ((39, -1, 4), (55, 8, 11))
SMEM_DONE_AT = 14
TAIL = (96, 120, 128)
G_RAW = 15
HEAD, HEAD_AT = 12, 2
RAW = (120, 128)

BULK, EARLY, LAST, BACK = range(4)


def _spans(t0, ends):
    return list(zip((t0,) + tuple(ends), ends))


def pallas_dist_max_ax1_xy_m2048_n1024_kernel(x: jax.Array):
    assert x.shape == (M, N) and 0 < OFF < TILES and UNIT == 2 * TILES
    assert all(t % TILES == 0 for t in TAIL + RAW)
    smem_p = _spans(OFF, [r[0] for r in SMEM])
    tail_p = _spans(smem_p[-1][1], TAIL)
    raw_p = _spans(HEAD, RAW)
    smem_slots = smem_p[-1][1] // TILES
    last_slot0 = TAIL[0] // TILES

    def body(x_hbm, out_ref, xbuf, rawbuf, bounce, part, r_part, s_early, r_early,
             s_last, r_last, s_back, r_back, main_sems, head_sems, tail_sems,
             reread_sem, smem_in_sems, smem_out_sems, send_sems, recv_sems,
             raw_send_sems, raw_recv_sems):
        my_y = lax.axis_index("y")
        nbr = (lax.axis_index("x"), 1 - my_y)

        def span(t0, t1):
            return pl.ds(t0, t1 - t0)

        def local(g, t0, t1, sem):
            return pltpu.make_async_copy(
                x_hbm.at[g, span(t0, t1)], xbuf.at[g, span(t0, t1)], sem)

        def main_copies(c):
            g0, u = STEPS[c]
            t0, sem = OFF + u * UNIT, main_sems.at[c]
            if t0 + UNIT <= GT:
                return [local(pl.ds(g0, WAYS), t0, t0 + UNIT, sem)]
            return [cp for g in range(g0, g0 + WAYS)
                    for cp in (local(g, t0, GT, sem), local(g + 1, 0, OFF, sem))]

        def remote(src, dst, send_sem, recv_sem):
            return pltpu.make_async_remote_copy(
                src_ref=src, dst_ref=dst, send_sem=send_sem, recv_sem=recv_sem,
                device_id=nbr, device_id_type=pl.DeviceIdType.MESH)

        def raw_copy(i):
            return remote(x_hbm.at[G_RAW, span(*raw_p[i])],
                          rawbuf.at[0, span(*raw_p[i])],
                          raw_send_sems.at[i], raw_recv_sems.at[i])

        def msg(k):
            src, dst = {BULK: (part, r_part), EARLY: (s_early, r_early),
                        LAST: (s_last, r_last), BACK: (s_back, r_back)}[k]
            return remote(src, dst, send_sems.at[k], recv_sems.at[k])

        heads = [local(G_RAW, 0, HEAD, head_sems.at[0]),
                 local(0, 0, OFF, head_sems.at[1])]
        tails = [local(G_TAIL, *p, tail_sems.at[i]) for i, p in enumerate(tail_p)]
        reread = local(G_RAW, HEAD, GT, reread_sem)
        to_smem, from_smem = [], []
        for i, (t0, t1) in enumerate(smem_p):
            stage = bounce.at[span(t0 - OFF, t1 - OFF)]
            to_smem.append(pltpu.make_async_copy(
                x_hbm.at[G_TAIL, span(t0, t1)], stage, smem_in_sems.at[i]))
            from_smem.append(pltpu.make_async_copy(
                stage, xbuf.at[G_TAIL, span(t0, t1)], smem_out_sems.at[i]))

        def start(copies):
            for cp in copies:
                cp.start()

        def wait(copies):
            for cp in copies:
                cp.wait()

        def smem_traffic(c):
            for i, (_, start_at, turn_at) in enumerate(SMEM):
                if c == turn_at:
                    to_smem[i].wait()
                    from_smem[i].start()
                if c == start_at:
                    to_smem[i].start()

        start(main_copies(0))
        smem_traffic(-1)
        barrier = pltpu.get_barrier_semaphore()
        pl.semaphore_signal(barrier, inc=1, device_id=nbr,
                            device_id_type=pl.DeviceIdType.MESH)

        @pl.when(my_y == 1)
        def _():
            pl.semaphore_wait(barrier, 1)
            for i in range(len(RAW)):
                raw_copy(i).start()

        for c in range(1, WINDOW):
            start(main_copies(c))

        diag = (lax.broadcasted_iota(jnp.int32, (SUB, LANES), 1)
                - lax.broadcasted_iota(jnp.int32, (SUB, LANES), 0))

        def fold(ref, g, t0, t1):
            out = []
            for s in range(t0 // TILES, pl.cdiv(t1, TILES)):
                tiles = ref[g, span(max(t0, s * TILES), min(t1, (s + 1) * TILES))]
                vs = [tiles[..., j, :, :] for j in range(tiles.shape[-3])]
                while len(vs) > 1:
                    vs = [jnp.maximum(*vs[i:i + 2]) if i + 1 < len(vs) else vs[i]
                          for i in range(0, len(vs), 2)]
                out.append((s, vs[0]))
            return out

        def place(acc, folded):
            for s, v in folded:
                acc = jnp.where(diag == s * SUB,
                                jnp.max(v, axis=-1, keepdims=True),
                                NEG if acc is None else acc)
            return acc

        def collapse(acc):
            return jnp.max(acc, axis=-2, keepdims=True)

        accs = None
        for c, (g0, u) in enumerate(STEPS):
            wait(main_copies(c))
            if c + WINDOW < len(STEPS):
                start(main_copies(c + WINDOW))
            elif c + WINDOW == len(STEPS):
                start(tails)
            smem_traffic(c)
            if c == HEAD_AT:
                start(heads)
            groups, t0, t1 = pl.ds(g0, WAYS), u * UNIT, (u + 1) * UNIT
            if t1 < GT:
                accs = place(accs, fold(xbuf, groups, max(t0, TILES), t1))
            else:
                if g0 == 0:
                    wait(heads)
                done = collapse(place(accs, fold(xbuf, groups, t0, t1)
                                      + fold(xbuf, groups, 0, TILES)))
                accs = None
                for k in range(WAYS):
                    part[:, pl.ds((g0 + k) * LANES, LANES)] = done[k]
                if g0 == 0:
                    part[:, pl.ds(G_TAIL * LANES, LANES)] = collapse(
                        place(None, fold(xbuf, G_RAW, 0, HEAD)))

                    @pl.when(my_y == 0)
                    def _():
                        pl.semaphore_wait(barrier, 1)
            if c == SMEM_DONE_AT:
                wait(from_smem)
                acc = place(None, fold(xbuf, G_TAIL, TILES, smem_slots * TILES))
        msg(BULK).start()

        tails[0].wait()
        early = collapse(place(
            acc, fold(xbuf, G_TAIL, 0, TILES)
            + fold(xbuf, G_TAIL, smem_slots * TILES, TAIL[0])))
        s_early[...] = early
        msg(EARLY).start()
        folded = []
        for cp, p in zip(tails[1:], tail_p[1:]):
            cp.wait()
            folded += fold(xbuf, G_TAIL, *p)
        last = collapse(place(None, folded))
        s_last[...] = last
        msg(LAST).start()

        reread.start()
        reread.wait()
        mine = collapse(place(None, fold(xbuf, G_RAW, 0, GT)))
        raw_row = pl.ds(G_RAW * LANES, LANES)

        @pl.when(my_y == 0)
        def _():
            s_back[...] = mine
            msg(BACK).start()
            acc = None
            for i, p in enumerate(raw_p):
                raw_copy(i).wait_recv()
                acc = place(acc, fold(rawbuf, 0, *p))
            out_ref[:, raw_row] = jnp.maximum(mine, collapse(acc))
            msg(BACK).wait_send()

        @pl.when(my_y == 1)
        def _():
            for i in range(len(RAW)):
                raw_copy(i).wait_send()
            msg(BACK).wait_recv()
            out_ref[:, raw_row] = jnp.maximum(mine, r_back[...])

        for k in (BULK, EARLY, LAST):
            msg(k).wait_send()

        msg(BULK).wait_recv()
        bulk = pl.ds(0, G_TAIL * LANES)
        out_ref[:, bulk] = jnp.maximum(part[:, bulk], r_part[:, bulk])
        out_ref[:, raw_row] = jnp.maximum(
            out_ref[:, raw_row], r_part[:, pl.ds(G_TAIL * LANES, LANES)])

        msg(EARLY).wait_recv()
        known = jnp.maximum(jnp.maximum(early, last), r_early[...])
        lane = lax.broadcasted_iota(jnp.int32, (1, LANES), 1)
        msg(LAST).wait_recv()
        theirs = known
        for l in range(last_slot0 * SUB, LANES):
            theirs = jnp.where(lane == l, r_last[0, l], theirs)
        out_ref[:, pl.ds(G_TAIL * LANES, LANES)] = jnp.maximum(known, theirs)

    x_tiles = x.reshape(GROUPS, SLOTS, SUB, TILES, LANES)
    x_tiles = x_tiles.transpose(0, 1, 3, 2, 4).reshape(GROUPS, GT, SUB, LANES)
    dma = pltpu.SemaphoreType.DMA
    out = pl.pallas_call(
        body,
        out_shape=jax.ShapeDtypeStruct((1, M), jnp.float32),
        in_specs=[pl.BlockSpec(memory_space=pl.ANY)],
        out_specs=pl.BlockSpec(memory_space=pltpu.VMEM),
        scratch_shapes=[
            pltpu.VMEM((GROUPS, GT, SUB, LANES), jnp.float32),
            pltpu.VMEM((1, GT, SUB, LANES), jnp.float32),
            pltpu.SMEM((smem_p[-1][1] - OFF, SUB, LANES), jnp.float32),
            pltpu.VMEM((1, M - LANES), jnp.float32),
            pltpu.VMEM((1, M - LANES), jnp.float32),
            pltpu.VMEM((1, LANES), jnp.float32),
            pltpu.VMEM((1, LANES), jnp.float32),
            pltpu.VMEM((1, LANES), jnp.float32),
            pltpu.SMEM((1, LANES), jnp.float32),
            pltpu.VMEM((1, LANES), jnp.float32),
            pltpu.VMEM((1, LANES), jnp.float32),
            dma((len(STEPS),)), dma((2,)), dma((len(TAIL),)), dma,
            dma((len(SMEM),)), dma((len(SMEM),)),
            dma((4,)), dma((4,)), dma((len(RAW),)), dma((len(RAW),)),
        ],
        compiler_params=pltpu.CompilerParams(
            collective_id=0,
            vmem_limit_bytes=32 * 1024 * 1024,
            disable_semaphore_checks=True,
        ),
    )(x_tiles)
    return out.reshape(M, 1)
```
